```python
import numpy as np

kernel_name = "dist_mean_ax0_shard0_i_m2048_n1024"

def setup_inputs():
    return {"x": np.random.randn(8192, 1024).astype(np.float32)}

def reference(x: np.ndarray) -> np.ndarray:
    return np.mean(x, axis=0, keepdims=True)
```

```python
import jax
import jax.numpy as jnp
from jax import lax
from jax.experimental import pallas as pl
from jax.experimental.pallas import tpu as pltpu

N_DEV = 4
ROWS = 8
FRONTS = 8
GROUPS = (192, 32, 16, 8, 4, 2, 2)


def pallas_dist_mean_ax0_shard0_i_m2048_n1024_kernel(x: jax.Array):
    m, n = x.shape
    n_pieces = m // ROWS
    assert sum(GROUPS) == n_pieces
    first = [sum(GROUPS[:g]) for g in range(len(GROUPS))]

    def body(x_hbm, out_ref, buf, slots, load_sems, send_sem, recv_sems):
        for g, size in enumerate(GROUPS):
            for k in range(first[g], first[g] + size):
                src = (k % FRONTS) * (n_pieces // FRONTS) + k // FRONTS
                pltpu.make_async_copy(
                    x_hbm.at[pl.ds(src * ROWS, ROWS)],
                    buf.at[pl.ds(k * ROWS, ROWS)],
                    load_sems.at[g],
                ).start(priority=k % 2)

        me = lax.axis_index("i")
        peer = {d: ((me + d) & (N_DEV - 1),) for d in (1, 2, 3)}
        barrier = pltpu.get_barrier_semaphore()
        for d in (1, 2, 3):
            pl.semaphore_signal(
                barrier, 1, device_id=peer[d], device_id_type=pl.DeviceIdType.MESH
            )

        acc = None
        for g, size in enumerate(GROUPS):
            if g == 2:
                pl.semaphore_wait(barrier, N_DEV - 1)
            blk = buf.at[pl.ds(first[g] * ROWS, size * ROWS)]
            pltpu.make_async_copy(blk, blk, load_sems.at[g]).wait()
            part = jnp.sum(blk[...].reshape(size, ROWS, n), axis=0)
            acc = part if acc is None else acc + part
        slots[0] = jnp.sum(acc * (1.0 / (m * N_DEV)), axis=0, keepdims=True)

        sends = {
            d: pltpu.make_async_remote_copy(
                slots.at[0],
                slots.at[d],
                send_sem,
                recv_sems.at[d - 1],
                device_id=peer[d],
                device_id_type=pl.DeviceIdType.MESH,
            )
            for d in (2, 1, 3)
        }
        for d in (2, 1, 3):
            sends[d].start()
        for d in (1, 3):
            sends[d].wait_recv()
        for d in (2, 1, 3):
            sends[d].wait_send()
        sends[2].wait_recv()
        out_ref[...] = (slots[0] + slots[2]) + (slots[1] + slots[3])

    return pl.pallas_call(
        body,
        out_shape=jax.ShapeDtypeStruct((1, n), jnp.float32),
        in_specs=[pl.BlockSpec(memory_space=pl.ANY)],
        out_specs=pl.BlockSpec(memory_space=pltpu.VMEM),
        scratch_shapes=[
            pltpu.VMEM((m, n), jnp.float32),
            pltpu.VMEM((N_DEV, 1, n), jnp.float32),
            pltpu.SemaphoreType.DMA((len(GROUPS),)),
            pltpu.SemaphoreType.DMA,
            pltpu.SemaphoreType.DMA((N_DEV - 1,)),
        ],
        compiler_params=pltpu.CompilerParams(
            collective_id=0,
            vmem_limit_bytes=32 * 1024 * 1024,
            disable_semaphore_checks=True,
        ),
    )(x)
```

```python
import jax
import jax.numpy as jnp
from jax import lax
from jax.experimental import pallas as pl
from jax.experimental.pallas import tpu as pltpu

N_DEV = 4
BAND = 8
FRONTS = 8
HEAD_START = 28
SIGNAL_AT = 64
LATE_COLS = 128
FULL_GROUPS = (32,)
SPLIT_GROUPS = (16, 6, 2)


def _tree_sum(xs):
    while len(xs) > 1:
        pairs = [a + b for a, b in zip(xs[0::2], xs[1::2])]
        xs = pairs + xs[2 * len(pairs):]
    return xs[0]


def pallas_dist_mean_ax0_shard0_i_m2048_n1024_kernel(x: jax.Array):
    m, n = x.shape
    n_bands = m // BAND
    n_split = sum(SPLIT_GROUPS)
    n_full = n_bands - n_split
    early_cols = n - LATE_COLS
    assert m % (BAND * FRONTS) == 0 and n_split % FRONTS == 0
    assert n_full > sum(FULL_GROUPS) and n_bands > SIGNAL_AT and early_cols > 0

    groups, first = [], 0
    for size in (n_full - sum(FULL_GROUPS), *FULL_GROUPS, *SPLIT_GROUPS):
        groups.append((first, size, n if first < n_full else early_cols))
        first += size

    def source_row(k):
        return (k % FRONTS * (n_bands // FRONTS) + k // FRONTS) * BAND

    def body(x_hbm, out_ref, buf, late_buf, sums, load_sems, send_sems, recv_sems):
        me = lax.axis_index("i")
        peers = {d: (lax.rem(me + d, N_DEV),) for d in range(1, N_DEV)}
        barrier = pltpu.get_barrier_semaphore()

        for g, (first, size, cols) in enumerate(groups):
            for k in range(first, first + size):
                pltpu.make_async_copy(
                    x_hbm.at[pl.ds(source_row(k), BAND), pl.ds(0, cols)],
                    buf.at[pl.ds(k * BAND, BAND), pl.ds(0, cols)],
                    load_sems.at[g],
                ).start(priority=1 if k < HEAD_START else k % 2)
                if k == SIGNAL_AT:
                    for peer in peers.values():
                        pl.semaphore_signal(
                            barrier,
                            1,
                            device_id=peer,
                            device_id_type=pl.DeviceIdType.MESH,
                        )
        late_sem = load_sems.at[len(groups)]
        rows = n_split // FRONTS * BAND
        for f in range(FRONTS):
            pltpu.make_async_copy(
                x_hbm.at[
                    pl.ds(source_row(n_full + f), rows), pl.ds(early_cols, LATE_COLS)
                ],
                late_buf.at[pl.ds(f * rows, rows)],
                late_sem,
            ).start(priority=1)

        early = late = None
        for g, (first, size, cols) in enumerate(groups):
            if g == 1:
                pl.semaphore_wait(barrier, N_DEV - 1)
            block = buf.at[pl.ds(first * BAND, size * BAND), pl.ds(0, cols)]
            pltpu.make_async_copy(block, block, load_sems.at[g]).wait()
            part = jnp.sum(block[...].reshape(size, BAND, cols), axis=0)
            early = part[:, :early_cols] if g == 0 else early + part[:, :early_cols]
            if cols == n:
                late = part[:, early_cols:] if g == 0 else late + part[:, early_cols:]

        def send(i, d, cols):
            copy = pltpu.make_async_remote_copy(
                sums.at[0, :, cols],
                sums.at[d, :, cols],
                send_sems.at[i],
                recv_sems.at[i],
                device_id=peers[d],
                device_id_type=pl.DeviceIdType.MESH,
            )
            copy.start()
            return copy

        sums[0, :, :early_cols] = jnp.sum(early, axis=0, keepdims=True)
        diagonal_early = send(0, 2, pl.ds(0, early_cols))

        pltpu.make_async_copy(late_buf, late_buf, late_sem).wait()
        late = _tree_sum(
            [late] + [late_buf[pl.ds(k * BAND, BAND), :] for k in range(n_split)]
        )
        sums[0, :, early_cols:] = jnp.sum(late, axis=0, keepdims=True)
        diagonal_late = send(1, 2, pl.ds(early_cols, LATE_COLS))
        right = send(2, 1, pl.ds(0, n))
        left = send(3, 3, pl.ds(0, n))

        right.wait()
        left.wait()
        neighbours = sums[1] + sums[3]
        diagonal_early.wait()
        diagonal_late.wait()
        out_ref[...] = ((sums[0] + sums[2]) + neighbours) * (1.0 / (m * N_DEV))

    return pl.pallas_call(
        body,
        out_shape=jax.ShapeDtypeStruct((1, n), jnp.float32),
        in_specs=[pl.BlockSpec(memory_space=pltpu.HBM)],
        out_specs=pl.BlockSpec(memory_space=pltpu.VMEM),
        scratch_shapes=[
            pltpu.VMEM((m, n), jnp.float32),
            pltpu.VMEM((n_split * BAND, LATE_COLS), jnp.float32),
            pltpu.VMEM((N_DEV, 1, n), jnp.float32),
            pltpu.SemaphoreType.DMA((len(groups) + 1,)),
            pltpu.SemaphoreType.DMA((4,)),
            pltpu.SemaphoreType.DMA((4,)),
        ],
        compiler_params=pltpu.CompilerParams(
            collective_id=0,
            disable_semaphore_checks=True,
        ),
    )(x)
```
